```python
import numpy as np

kernel_name = "dist_mean_ax1_xy_m1024_n512"

def setup_inputs():
    return {"x": np.random.randn(2048, 1024).astype(np.float32)}

def reference(x: np.ndarray) -> np.ndarray:
    return np.mean(x, axis=1, keepdims=True)
```

```python
import jax
import jax.numpy as jnp
from jax import lax
from jax.experimental import pallas as pl
from jax.experimental.pallas import tpu as pltpu

_LANES = 128
_SUB = 8
_NT_DIMS = (((1,), (1,)), ((), ()))
_MESH = pl.DeviceIdType.MESH


def _compiler_params():
    try:
        return pltpu.CompilerParams(collective_id=0,
                                    disable_semaphore_checks=True)
    except TypeError:
        return pltpu.CompilerParams(collective_id=0)


def _tree_add(vals):
    while len(vals) > 1:
        nxt = [vals[i] + vals[i + 1] for i in range(0, len(vals) - 1, 2)]
        if len(vals) % 2:
            nxt.append(vals[-1])
        vals = nxt
    return vals[0]


def pallas_dist_mean_ax1_xy_m1024_n512_kernel(
    x: jax.Array,
):
    m, n = x.shape
    assert m % _LANES == 0 and n % _LANES == 0 and m >= 3 * _LANES
    scale = 1.0 / (2 * n)

    last = m - _LANES
    mxu_rows = 32
    xlu_rows = 48
    crit = mxu_rows + xlu_rows
    raw_rows = _LANES - crit
    final = _SUB
    half = (m // (2 * _LANES)) * _LANES

    head = [(0, half), (half, last - half)]
    chunks = head + [(last + final, crit - final), (last, final),
                     (last + crit, raw_rows)]
    xlu_offs = list(range(mxu_rows, crit, _SUB))

    def fold(v):
        return _tree_add([v[:, j:j + _LANES] for j in range(0, n, _LANES)])

    def row_sums(p):
        w = jnp.full((_SUB, _LANES), scale, jnp.float32)
        r = lax.dot_general(w, p, _NT_DIMS, preferred_element_type=jnp.float32)
        return r[0:1, :]

    def body(x_hbm, o_ref, xbuf, raw_buf, s_head, s_last, r_head, r_last,
             load_sems, send_sems, recv_sems):
        loads = [
            pltpu.make_async_copy(
                x_hbm.at[pl.ds(a, s)], xbuf.at[pl.ds(a, s)], load_sems.at[i])
            for i, (a, s) in enumerate(chunks)
        ]
        loads[0].start()

        peer = (lax.axis_index("x"), 1 - lax.axis_index("y"))
        barrier = pltpu.get_barrier_semaphore()
        pl.semaphore_signal(barrier, inc=1, device_id=peer,
                            device_id_type=_MESH)
        for c in loads[1:4]:
            c.start()

        def send(k, src, dst):
            return pltpu.make_async_remote_copy(
                src_ref=src, dst_ref=dst,
                send_sem=send_sems.at[k], recv_sem=recv_sems.at[k],
                device_id=peer, device_id_type=_MESH)

        send_head = send(0, s_head, r_head)
        send_last = send(1, s_last, r_last)
        send_raw = send(2, x_hbm.at[pl.ds(last + crit, raw_rows)], raw_buf)

        diag = (lax.broadcasted_iota(jnp.int32, (_SUB, _LANES), 1)
                - lax.broadcasted_iota(jnp.int32, (_SUB, _LANES), 0))
        masks = [diag == o for o in xlu_offs]

        pl.semaphore_wait(barrier, 1)
        send_raw.start()

        for i, (a, s) in enumerate(head):
            loads[i].wait()
            for j in range(a, a + s, _LANES):
                s_head[:, j:j + _LANES] = row_sums(fold(xbuf[j:j + _LANES, :]))
        send_head.start()

        loads[2].wait()
        p_mid = fold(xbuf[last + final:last + mxu_rows, :])
        p_xlu = [fold(xbuf[last + o:last + o + _SUB, :]) * scale
                 for o in xlu_offs]
        loads[3].wait()
        p_fin = fold(xbuf[last:last + final, :])
        red = [jnp.broadcast_to(jnp.sum(p, axis=1, keepdims=True),
                                (_SUB, _LANES)) for p in p_xlu]
        placed = [
            jnp.where(masks[g + 1], red[g + 1],
                      jnp.where(masks[g], red[g], 0.0))
            for g in range(0, len(red), 2)
        ]
        s_last[...] = jnp.sum(_tree_add(placed), axis=0, keepdims=True)
        s_last[:, 0:mxu_rows] = row_sums(
            jnp.concatenate([p_fin, p_mid], axis=0))
        send_last.start()

        loads[4].start()
        loads[4].wait()
        send_raw.wait_recv()
        p_raw = fold(xbuf[last + crit:m, :]) + fold(raw_buf[...])
        mine = s_last[...] + row_sums(jnp.concatenate(
            [jnp.zeros((crit, _LANES), jnp.float32), p_raw], axis=0))

        send_raw.wait_send()
        send_head.wait_send()
        send_head.wait_recv()
        o_ref[:, 0:last] = s_head[...] + r_head[...]
        send_last.wait_send()
        send_last.wait_recv()
        o_ref[:, last:m] = mine + r_last[...]

    out = pl.pallas_call(
        body,
        out_shape=jax.ShapeDtypeStruct((1, m), jnp.float32),
        in_specs=[pl.BlockSpec(memory_space=pl.ANY)],
        out_specs=pl.BlockSpec(memory_space=pltpu.VMEM),
        scratch_shapes=[
            pltpu.VMEM((m, n), jnp.float32),
            pltpu.VMEM((raw_rows, n), jnp.float32),
            pltpu.VMEM((1, last), jnp.float32),
            pltpu.VMEM((1, _LANES), jnp.float32),
            pltpu.VMEM((1, last), jnp.float32),
            pltpu.VMEM((1, _LANES), jnp.float32),
            pltpu.SemaphoreType.DMA((len(chunks),)),
            pltpu.SemaphoreType.DMA((3,)),
            pltpu.SemaphoreType.DMA((3,)),
        ],
        compiler_params=_compiler_params(),
    )(x)
    return out.reshape(m, 1)
```
